```python
import numpy as np

kernel_name = "dist_mean_ax1_xy_m4096_n1024"

def setup_inputs():
    return {"x": np.random.randn(8192, 2048).astype(np.float32)}

def reference(x: np.ndarray) -> np.ndarray:
    return np.mean(x, axis=1, keepdims=True)
```

```python
import jax
import jax.numpy as jnp
from jax import lax
from jax.experimental import pallas as pl
from jax.experimental.pallas import tpu as pltpu

LANES = 128
BLOCK = 256
RAW = (128, 96)


def pallas_dist_mean_ax1_xy_m4096_n1024_kernel(x: jax.Array):
    m, n = x.shape
    half = m // 2
    scale = 1.0 / (2 * n)
    mesh_id = pl.DeviceIdType.MESH

    raw_rows = sum(RAW)
    local_rows = half - raw_rows
    raw_base = local_rows // LANES * LANES
    raw_pad = half - raw_base
    sent = -(-local_rows // LANES) * LANES

    late_chunks = [(0, 1536), (1536, 384), (1920, 128)]
    early_chunks = [(0, 1024), (1024, raw_base - 1280), (raw_base, raw_pad),
                    (raw_base - 256, 128), (raw_base - 128, 128)]
    for chunks in (late_chunks, early_chunks):
        assert sorted(r for o, s in chunks for r in range(o, o + s)) == list(range(half))
    n_chunks = max(len(late_chunks), len(early_chunks))

    def body(x_hbm, out_ref, buf, part, recv, raw_buf, raw_sum,
             in_sems, part_send, part_recv, raw_send, raw_recv, out_send, out_recv):
        my_y = lax.axis_index("y")
        partner = (lax.axis_index("x"), 1 - my_y)
        barrier = pltpu.get_barrier_semaphore()

        def remote(src, dst, send_sem, recv_sem):
            return pltpu.make_async_remote_copy(
                src, dst, send_sem, recv_sem, device_id=partner, device_id_type=mesh_id)

        def row_sums(src, src0, dst, dst0, rows):
            def block(s, d, b):
                dst[:, pl.ds(d, b)] = jnp.sum(src[pl.ds(s, b), :], axis=1).reshape(1, b)

            steps, done = rows // BLOCK, 0
            if steps > 1:
                def step(j, carry):
                    block(pl.multiple_of(src0 + j * BLOCK, LANES),
                          pl.multiple_of(dst0 + j * BLOCK, LANES), BLOCK)
                    return carry

                lax.fori_loop(0, steps, step, 0)
                done = steps * BLOCK
            for r in range(done, rows, LANES):
                block(src0 + r, dst0 + r, LANES)

        raw_copies, off = [], 0
        for k, rows in enumerate(RAW):
            raw_copies.append(remote(
                x_hbm.at[pl.ds(local_rows + off, rows)],
                raw_buf.at[pl.ds(raw_pad - raw_rows + off, rows)],
                raw_send.at[k], raw_recv.at[k]))
            off += rows

        def run(late):
            own0, other0 = (half, 0) if late else (0, half)
            chunks = late_chunks if late else early_chunks
            first_rows = local_rows if late else half
            n_send, n_recv = (sent, half) if late else (half, sent)

            first = pltpu.make_async_copy(
                x_hbm.at[pl.ds(other0, first_rows)], buf.at[pl.ds(0, first_rows)],
                in_sems.at[0])
            second = [
                pltpu.make_async_copy(
                    x_hbm.at[pl.ds(own0 + off, rows)], buf.at[pl.ds(half + off, rows)],
                    in_sems.at[1 + i])
                for i, (off, rows) in enumerate(chunks)]

            first.start()
            pl.semaphore_signal(barrier, inc=1, device_id=partner, device_id_type=mesh_id)
            for copy in second:
                copy.start()
            if late:
                pl.semaphore_wait(barrier, 1)
                raw_copies[0].start()
                buf[pl.ds(first_rows, sent - first_rows), :] = jnp.zeros(
                    (sent - first_rows, n), jnp.float32)
            else:
                raw_buf[pl.ds(0, raw_pad - raw_rows), :] = jnp.zeros(
                    (raw_pad - raw_rows, n), jnp.float32)

            first.wait()
            row_sums(buf, 0, part, 0, n_send)
            if not late:
                pl.semaphore_wait(barrier, 1)
            part_out = remote(part.at[:, pl.ds(0, n_send)], recv.at[:, pl.ds(0, n_send)],
                              part_send, part_recv)
            part_out.start()
            sends = [part_out]
            if late:
                for copy in raw_copies[1:]:
                    copy.start()
                sends += raw_copies

            for i, (off, rows) in enumerate(chunks):
                second[i].wait()
                row_sums(buf, half + off, part, half + off, rows)
                if i == 0:
                    remote(part.at[:, pl.ds(0, n_recv)], recv.at[:, pl.ds(0, n_recv)],
                           part_send, part_recv).wait_recv()
                if not late and off == raw_base:
                    for copy in raw_copies:
                        copy.wait_recv()
                    row_sums(raw_buf, 0, raw_sum, 0, raw_pad)
                    both = sent - raw_base
                    recv[:, pl.ds(raw_base, both)] = (
                        recv[:, pl.ds(raw_base, both)] + raw_sum[:, pl.ds(0, both)])
                    recv[:, pl.ds(sent, half - sent)] = raw_sum[:, pl.ds(both, half - sent)]
                means = out_ref.at[:, pl.ds(own0 + off, rows)]
                means[...] = (part[:, pl.ds(half + off, rows)] + recv[:, pl.ds(off, rows)]) * scale
                publish = remote(means, means, out_send.at[i], out_recv)
                publish.start()
                sends.append(publish)

            for copy in sends:
                copy.wait_send()
            theirs = out_ref.at[:, pl.ds(other0, half)]
            pltpu.make_async_copy(theirs, theirs, out_recv).wait()

        @pl.when(my_y == 0)
        def _():
            run(late=False)

        @pl.when(my_y == 1)
        def _():
            run(late=True)

    out = pl.pallas_call(
        body,
        out_shape=jax.ShapeDtypeStruct((1, m), jnp.float32),
        in_specs=[pl.BlockSpec(memory_space=pl.ANY)],
        out_specs=pl.BlockSpec(memory_space=pltpu.VMEM),
        scratch_shapes=[
            pltpu.VMEM((m, n), jnp.float32),
            pltpu.VMEM((1, m), jnp.float32),
            pltpu.VMEM((1, half), jnp.float32),
            pltpu.VMEM((raw_pad, n), jnp.float32),
            pltpu.VMEM((1, raw_pad), jnp.float32),
            pltpu.SemaphoreType.DMA((1 + n_chunks,)),
            pltpu.SemaphoreType.DMA,
            pltpu.SemaphoreType.DMA,
            pltpu.SemaphoreType.DMA((len(RAW),)),
            pltpu.SemaphoreType.DMA((len(RAW),)),
            pltpu.SemaphoreType.DMA((n_chunks,)),
            pltpu.SemaphoreType.DMA,
        ],
        compiler_params=pltpu.CompilerParams(
            collective_id=0,
            vmem_limit_bytes=64 * 1024 * 1024,
            disable_bounds_checks=True,
            disable_semaphore_checks=True,
        ),
    )(x)
    return out.reshape(m, 1)
```
